```python
import numpy as np

kernel_name = "dist_f_of_ar_i_m4096_n1024"

def setup_inputs():
    t = np.random.randn(16384, 1024).astype(np.float32)
    return {"t": t}

def reference(t: np.ndarray) -> np.ndarray:
    s = t.reshape(4, 4096, 1024).sum(axis=0)
    r = np.maximum(s, 0.0)
    return np.tanh(s) * s * s + r * r * r
```

```python
import jax
import jax.numpy as jnp
from jax import lax
from jax.experimental import pallas as pl
from jax.experimental.pallas import tpu as pltpu

N_DEV = 4
LINKS = ((1, 3), (3, 1))
N_GROUPS = len(LINKS)
TILE = 16
HEAD = ((0, 16), (16, 64), (64, 192), (192, None))
N_PARTS = 2


def _f(s):
    r = jnp.maximum(s, 0.0)
    return jnp.tanh(s) * s * s + r * r * r


def pallas_dist_f_of_ar_i_m4096_n1024_kernel(
    t: jax.Array,
):
    m, n = t.shape
    rows = m // (N_GROUPS * N_DEV)
    part = rows // N_PARTS
    head = tuple((lo, (rows if hi is None else hi) - lo) for lo, hi in HEAD)
    f32, bf16 = jnp.float32, jnp.bfloat16

    def body(
        x_hbm, out,
        x_far, x_near, x_pair, x_mine,
        tx_far, tx_near, tx_pair,
        rx_far, rx_near, rx_pair,
        head_sems, load_sems, send_sem,
        far_sem, near_sem, pair_sems, gather_sems,
    ):
        me = lax.axis_index("i")

        barrier = pltpu.get_barrier_semaphore()
        for d in (1, 3):
            pl.semaphore_signal(
                barrier, 1, device_id=(me ^ d,), device_id_type=pl.DeviceIdType.MESH
            )

        def block(g, owner, lo=0, size=rows):
            return pl.ds(pl.multiple_of((owner * N_GROUPS + g) * rows + lo, TILE), size)

        def load(g, owner, dst, sem, lo=0, size=rows):
            pltpu.make_async_copy(
                x_hbm.at[block(g, owner, lo, size)], dst.at[g, pl.ds(lo, size)], sem
            ).start()

        sends = []

        def send(src, dst, recv_sem, d):
            copy = pltpu.make_async_remote_copy(
                src, dst, send_sem, recv_sem,
                device_id=(me ^ d,), device_id_type=pl.DeviceIdType.MESH,
            )
            copy.start()
            sends.append(copy)

        def wait_filled(buf, sem):
            pltpu.make_async_copy(buf, buf, sem).wait()

        def for_tiles(size, step):
            @pl.loop(0, size // TILE)
            def _(k):
                for g in range(N_GROUPS):
                    step(g, pl.multiple_of(k * TILE, TILE))

        for c, (lo, size) in enumerate(head):
            for g in range(N_GROUPS):
                load(g, me ^ 2, x_far, head_sems.at[c], lo, size)
        for g, (d1, d2) in enumerate(LINKS):
            load(g, me ^ d1, x_near, load_sems.at[0])
        for g, (d1, d2) in enumerate(LINKS):
            load(g, me ^ d2, x_pair, load_sems.at[1])
        for g in range(N_GROUPS):
            load(g, me, x_mine, load_sems.at[2])

        for c, (lo, size) in enumerate(head):
            wait_filled(x_far.at[:, pl.ds(lo, size)], head_sems.at[c])

            def round_far(g, i, lo=lo):
                tile = pl.ds(lo + i, TILE)
                tx_far[g, tile, :] = x_far[g, tile, :].astype(bf16)

            for_tiles(size, round_far)
            if c == 0:
                pl.semaphore_wait(barrier, 2)
            for g, (d1, d2) in enumerate(LINKS):
                piece = pl.ds(lo, size)
                send(tx_far.at[g, piece], rx_far.at[g, piece], far_sem, d1)

        wait_filled(x_near, load_sems.at[0])

        def round_near(g, i):
            tile = pl.ds(i, TILE)
            tx_near[g, tile, :] = x_near[g, tile, :].astype(bf16)

        for_tiles(rows, round_near)
        for g, (d1, d2) in enumerate(LINKS):
            send(tx_near.at[g], rx_near.at[g], near_sem, d1)

        wait_filled(x_pair, load_sems.at[1])
        wait_filled(rx_far, far_sem)

        def add_pair(g, i):
            tile = pl.ds(i, TILE)
            s = x_pair[g, tile, :] + rx_far[g, tile, :].astype(f32)
            tx_pair[g, tile, :] = s.astype(bf16)

        for_tiles(rows, add_pair)
        for h in range(N_PARTS):
            for g, (d1, d2) in enumerate(LINKS):
                send(
                    tx_pair.at[g, pl.ds(h * part, part)], rx_pair.at[h, g],
                    pair_sems.at[h], d2,
                )

        wait_filled(x_mine, load_sems.at[2])
        wait_filled(rx_near, near_sem)
        for h in range(N_PARTS):
            wait_filled(rx_pair.at[h], pair_sems.at[h])

            def finish(g, i, h=h):
                tile = pl.ds(h * part + i, TILE)
                s = x_mine[g, tile, :] + rx_near[g, tile, :].astype(f32)
                s = s + rx_pair[h, g, pl.ds(i, TILE), :].astype(f32)
                out[block(g, me, h * part + i, TILE), :] = _f(s).astype(bf16)

            for_tiles(part, finish)
            for g, (d1, d2) in enumerate(LINKS):
                piece = out.at[block(g, me, h * part, part)]
                send(piece, piece, gather_sems.at[g], d2)

        for g, (d1, d2) in enumerate(LINKS):
            mine = out.at[block(g, me)]
            send(mine, mine, gather_sems.at[N_GROUPS + g], d1)

        for g, (d1, d2) in enumerate(LINKS):
            theirs = out.at[block(g, me ^ d2)]
            wait_filled(theirs, gather_sems.at[g])
            send(theirs, theirs, gather_sems.at[2 * N_GROUPS + g], d1)

        for g, (d1, d2) in enumerate(LINKS):
            wait_filled(out.at[block(g, me ^ d1)], gather_sems.at[N_GROUPS + g])
        for copy in sends:
            copy.wait_send()
        for g in range(N_GROUPS):
            wait_filled(out.at[block(g, me ^ 2)], gather_sems.at[2 * N_GROUPS + g])

    stage = (N_GROUPS, rows, n)
    out = pl.pallas_call(
        body,
        out_shape=pltpu.VMEM((m, n), bf16),
        in_specs=[pl.BlockSpec(memory_space=pltpu.HBM)],
        out_specs=pl.BlockSpec(memory_space=pltpu.VMEM),
        scratch_shapes=[
            *[pltpu.VMEM(stage, f32)] * 4,
            *[pltpu.VMEM(stage, bf16)] * 5,
            pltpu.VMEM((N_PARTS, N_GROUPS, part, n), bf16),
            pltpu.SemaphoreType.DMA((len(head),)),
            pltpu.SemaphoreType.DMA((3,)),
            pltpu.SemaphoreType.DMA,
            pltpu.SemaphoreType.DMA,
            pltpu.SemaphoreType.DMA,
            pltpu.SemaphoreType.DMA((N_PARTS,)),
            pltpu.SemaphoreType.DMA((3 * N_GROUPS,)),
        ],
        compiler_params=pltpu.CompilerParams(
            collective_id=0, vmem_limit_bytes=48 * 2**20
        ),
    )(t)
    return out.astype(t.dtype)
```

```python
import jax
import jax.numpy as jnp
from jax import lax
from jax.experimental import pallas as pl
from jax.experimental.pallas import tpu as pltpu

N_DEV = 4
LINKS = ((1, 3), (3, 1))
N_GROUPS = len(LINKS)
TILE = 16
HEAD = (0, 16, 64, 192)
N_PARTS = 2


def _f(s):
    r = jnp.maximum(s, 0.0)
    return jnp.tanh(s) * s * s + r * r * r


def pallas_dist_f_of_ar_i_m4096_n1024_kernel(
    t: jax.Array,
):
    m, n = t.shape
    rows = m // (N_DEV * N_GROUPS)
    part = rows // N_PARTS
    head = [(lo, hi - lo) for lo, hi in zip(HEAD, (*HEAD[1:], rows))]
    f32, bf16 = jnp.float32, jnp.bfloat16

    def body(
        x_hbm, out,
        x_far, x_near, x_pair, x_mine,
        tx_far, tx_near, tx_pair,
        rx_far, rx_near, rx_pair,
        load_sems, send_sem,
        far_sem, near_sem, pair_sems, relay_sems, direct_sems, diagonal_sems,
    ):
        me = lax.axis_index("i")

        barrier = pltpu.get_barrier_semaphore()
        for d in (1, 3):
            pl.semaphore_signal(
                barrier, 1, device_id=(me ^ d,), device_id_type=pl.DeviceIdType.MESH
            )

        def block(g, owner, lo=0, size=rows):
            return pl.ds(pl.multiple_of((owner * N_GROUPS + g) * rows + lo, TILE), size)

        def load(g, owner, dst, sem, lo=0, size=rows):
            pltpu.make_async_copy(
                x_hbm.at[block(g, owner, lo, size)], dst.at[g, pl.ds(lo, size)], sem
            ).start()

        sends = []

        def send(src, dst, recv_sem, d):
            copy = pltpu.make_async_remote_copy(
                src, dst, send_sem, recv_sem,
                device_id=(me ^ d,), device_id_type=pl.DeviceIdType.MESH,
            )
            copy.start()
            sends.append(copy)

        def wait_filled(buf, sem):
            pltpu.make_async_copy(buf, buf, sem).wait()

        def for_tiles(size, step):
            @pl.loop(0, size // TILE)
            def _(k):
                for g in range(N_GROUPS):
                    step(g, pl.multiple_of(k * TILE, TILE))

        for c, (lo, size) in enumerate(head):
            for g in range(N_GROUPS):
                load(g, me ^ 2, x_far, load_sems.at[c], lo, size)
        for c, (lo, size) in enumerate(head):
            piece = pl.ds(lo, size)
            wait_filled(x_far.at[:, piece], load_sems.at[c])

            def round_far(g, i, lo=lo):
                tile = pl.ds(lo + i, TILE)
                tx_far[g, tile, :] = x_far[g, tile, :].astype(bf16)

            for_tiles(size, round_far)
            if c == 0:
                pl.semaphore_wait(barrier, 2)
            for g, (d1, d2) in enumerate(LINKS):
                send(tx_far.at[g, piece], rx_far.at[g, piece], far_sem, d1)

        for g, (d1, d2) in enumerate(LINKS):
            load(g, me ^ d1, x_near, load_sems.at[0])
        wait_filled(x_near, load_sems.at[0])
        for g, (d1, d2) in enumerate(LINKS):
            load(g, me ^ d2, x_pair, load_sems.at[1])
            load(g, me, x_mine, load_sems.at[2])

        def round_near(g, i):
            tile = pl.ds(i, TILE)
            tx_near[g, tile, :] = x_near[g, tile, :].astype(bf16)

        for_tiles(rows, round_near)
        for g, (d1, d2) in enumerate(LINKS):
            send(tx_near.at[g], rx_near.at[g], near_sem, d1)

        wait_filled(x_pair, load_sems.at[1])
        wait_filled(rx_far, far_sem)

        def add_pair(g, i):
            tile = pl.ds(i, TILE)
            s = x_pair[g, tile, :] + rx_far[g, tile, :].astype(f32)
            tx_pair[g, tile, :] = s.astype(bf16)

        for_tiles(rows, add_pair)
        for h in range(N_PARTS):
            for g, (d1, d2) in enumerate(LINKS):
                piece = tx_pair.at[g, pl.ds(h * part, part)]
                send(piece, rx_pair.at[h, g], pair_sems.at[h], d2)

        wait_filled(x_mine, load_sems.at[2])
        wait_filled(rx_near, near_sem)
        for h in range(N_PARTS):
            wait_filled(rx_pair.at[h], pair_sems.at[h])

            def finish(g, i, h=h):
                tile = pl.ds(h * part + i, TILE)
                s = x_mine[g, tile, :] + rx_near[g, tile, :].astype(f32)
                s = s + rx_pair[h, g, pl.ds(i, TILE), :].astype(f32)
                out[block(g, me, h * part + i, TILE), :] = _f(s).astype(bf16)

            for_tiles(part, finish)
            for g, (d1, d2) in enumerate(LINKS):
                piece = out.at[block(g, me, h * part, part)]
                send(piece, piece, relay_sems.at[g], d2)

        for g, (d1, d2) in enumerate(LINKS):
            mine = out.at[block(g, me)]
            send(mine, mine, direct_sems.at[g], d1)

        for g, (d1, d2) in enumerate(LINKS):
            theirs = out.at[block(g, me ^ d2)]
            wait_filled(theirs, relay_sems.at[g])
            send(theirs, theirs, diagonal_sems.at[g], d1)

        for g, (d1, d2) in enumerate(LINKS):
            wait_filled(out.at[block(g, me ^ d1)], direct_sems.at[g])
        for copy in sends:
            copy.wait_send()
        for g in range(N_GROUPS):
            wait_filled(out.at[block(g, me ^ 2)], diagonal_sems.at[g])

    stage = (N_GROUPS, rows, n)
    gathered = pl.pallas_call(
        body,
        out_shape=pltpu.VMEM((m, n), bf16),
        in_specs=[pl.BlockSpec(memory_space=pltpu.HBM)],
        out_specs=pl.BlockSpec(memory_space=pltpu.VMEM),
        scratch_shapes=[
            *[pltpu.VMEM(stage, f32)] * 4,
            *[pltpu.VMEM(stage, bf16)] * 5,
            pltpu.VMEM((N_PARTS, N_GROUPS, part, n), bf16),
            pltpu.SemaphoreType.DMA((len(head),)),
            pltpu.SemaphoreType.DMA,
            pltpu.SemaphoreType.DMA,
            pltpu.SemaphoreType.DMA,
            pltpu.SemaphoreType.DMA((N_PARTS,)),
            *[pltpu.SemaphoreType.DMA((N_GROUPS,))] * 3,
        ],
        compiler_params=pltpu.CompilerParams(
            collective_id=0, vmem_limit_bytes=48 * 2**20
        ),
    )(t)
    return gathered.astype(t.dtype)
```
